```python
import numpy as np

kernel_name = "dist_matmul_relu_kshard_i_m1024_n1024_k512"

def setup_inputs():
    A = np.random.randn(1024, 2048).astype(np.float32)
    B = np.random.randn(2048, 1024).astype(np.float32)
    return {"A": A, "B": B}

def reference(A: np.ndarray, B: np.ndarray) -> np.ndarray:
    z = A @ B
    return np.maximum(z, 0.0)
```

```python
import jax
import jax.numpy as jnp
from jax import lax
from jax.experimental import pallas as pl
from jax.experimental.pallas import tpu as pltpu

M = 1024
N = 1024
KS = 512
QR = 256
ER = 128
GW = 256
NG = N // GW
PR = 120
PW = GW // 2

_P_ODD = dict(
    loads=(('B', 0, 128), ('A', 0, 0, 32), ('A', 0, 32, 80), ('A', 0, 80, 128),
           ('B', 128, 256), ('A', 1, 0, 128), ('A', 0, 128, 256), ('A', 1, 128, 256)),
    steps=((0, 0, 32, 0, 128), (0, 32, 80, 0, 128), (0, 80, 128, 0, 128),
           (0, 0, 128, 128, 256), (1, 0, 128, 0, 256), (0, 128, 256, 0, 256),
           (1, 128, 256, 0, 256)),
)
_P_EVEN = dict(
    loads=(('B', 0, 128), ('A', 0, 0, 64), ('A', 1, 0, 64), ('A', 0, 64, 128),
           ('A', 1, 64, 128), ('B', 128, 256), ('A', 0, 128, 256), ('A', 1, 128, 256)),
    steps=((0, 0, 64, 0, 128), (1, 0, 64, 0, 128), (0, 64, 128, 0, 128),
           (1, 64, 128, 0, 128), (0, 0, 128, 128, 256), (1, 0, 128, 128, 256),
           (0, 128, 256, 0, 256), (1, 128, 256, 0, 256)),
)
_DEFER0 = 4
_COMMON_B = ((256, 384), (384, 512), (512, 768), (768, 1024))
_NLS = max(len(_P_ODD['loads']), len(_P_EVEN['loads']))
_NCB = len(_COMMON_B)

_BF = jnp.bfloat16
_F32 = jnp.float32
_U32 = jnp.uint32
_MESH = pl.DeviceIdType.MESH


def _body(a_hbm, b_hbm, o_ref,
          a_f32, b_f32, a_bf, b_bf, s1, r1, acc, s2, r2, pk_own, pk_a, pk_b,
          lsem, ready, ssem, rs1, rs2, rs3a, rs3b):
    i = lax.axis_index("i")
    x = i >> 1
    y = (i ^ x) & 1
    py = i ^ 1
    px = 3 - i
    isx = x == 1

    def sel(h0, h1, role):
        lst = (h0, h1)
        return jnp.where(isx, lst[1 - role], lst[role])

    base = [sel(0, 2 * QR, r) for r in range(2)]
    ac = [sel(y, x, r) for r in range(2)]
    bc = [sel(x, y, r) for r in range(2)]
    t13 = [sel(py, px, r) for r in range(2)]
    t2 = [sel(px, py, r) for r in range(2)]
    rr13 = x
    rr2 = 1 - x

    def grow(slot, e):
        r = slot % 2
        q = ac[r] if slot >= 2 else 1 - ac[r]
        ee = bc[r] if e == 1 else 1 - bc[r]
        return pl.multiple_of(base[r] + q * QR + ee * ER, ER)

    def a_copy(slot, r0, r1_, sem):
        e = r0 // ER
        assert (r1_ - 1) // ER == e
        return pltpu.make_async_copy(
            a_hbm.at[pl.ds(grow(slot, e) + (r0 - e * ER), r1_ - r0), :],
            a_f32.at[pl.ds(slot * QR + r0, r1_ - r0), :], sem)

    def b_copy(c0, c1, sem):
        return pltpu.make_async_copy(
            b_hbm.at[:, pl.ds(c0, c1 - c0)], b_f32.at[:, pl.ds(c0, c1 - c0)], sem)

    def common_loads():
        cps = [b_copy(c0, c1, lsem.at[_NLS + k]) for k, (c0, c1) in enumerate(_COMMON_B)]
        k = _NLS + _NCB
        for slot in (2, 3):
            for e in range(2):
                cps.append(a_copy(slot, e * ER, (e + 1) * ER, lsem.at[k]))
                k += 1
        return cps

    def rdma1(role, r0, r1_, c0, c1):
        g = c0 // GW
        assert (c1 - 1) // GW == g
        return pltpu.make_async_remote_copy(
            s1.at[role, pl.ds(r0, r1_ - r0), pl.ds(c0, c1 - c0)],
            r1.at[rr13, pl.ds(r0, r1_ - r0), pl.ds(c0, c1 - c0)],
            ssem.at[0], rs1.at[rr13 * NG + g],
            device_id=(t13[role],), device_id_type=_MESH)

    bar = pltpu.get_barrier_semaphore()

    def signal_neighbours(sem):
        for nb in (py, px):
            pl.semaphore_signal(sem, inc=1, device_id=(nb,), device_id_type=_MESH)

    def startup(prog, odd):
        loads, steps = prog['loads'], prog['steps']

        def load(k):
            l = loads[k]
            if l[0] == 'B':
                return b_copy(l[1], l[2], lsem.at[k])
            return a_copy(l[1], l[2], l[3], lsem.at[k])

        for k in range(len(loads)):
            load(k).start()
        for cp in common_loads():
            cp.start()

        if odd:
            signal_neighbours(bar)
        else:
            @pl.when(i == 0)
            def _():
                signal_neighbours(bar)

            @pl.when(i == 2)
            def _():
                pl.semaphore_wait(bar, 2)
                signal_neighbours(ready)

        loaded = set()

        def need(role, r0, r1_, c0, c1):
            last = -1
            for k, l in enumerate(loads):
                if l[0] == 'B' and l[1] < c1 and l[2] > c0:
                    last = max(last, k)
                if l[0] == 'A' and l[1] == role and l[2] < r1_ and l[3] > r0:
                    last = max(last, k)
            for k in range(last + 1):
                if k in loaded:
                    continue
                loaded.add(k)
                l = loads[k]
                load(k).wait()
                if l[0] == 'B':
                    b_bf[:, l[1]:l[2]] = b_f32[:, l[1]:l[2]].astype(_BF)
                else:
                    o = l[1] * QR
                    a_bf[o + l[2]:o + l[3], :] = a_f32[o + l[2]:o + l[3], :].astype(_BF)

        shaken = [False, False]
        for si, (role, r0, r1_, c0, c1) in enumerate(steps):
            need(role, r0, r1_, c0, c1)
            res = jnp.dot(a_bf[role * QR + r0:role * QR + r1_, :], b_bf[:, c0:c1],
                          preferred_element_type=_F32)
            s1[role, r0:r1_, c0:c1] = res.astype(_BF)
            if odd:
                if not shaken[role]:
                    shaken[role] = True
                    if role == 0:
                        pl.semaphore_wait(bar, 1)
                    else:
                        pl.semaphore_wait(ready, 1)
                rdma1(role, r0, r1_, c0, c1).start()
            elif si < _DEFER0:
                @pl.when(i == 2)
                def _():
                    rdma1(role, r0, r1_, c0, c1).start()

                if si == _DEFER0 - 1:
                    @pl.when(i == 0)
                    def _():
                        pl.semaphore_wait(bar, 2)
                        for st in steps[:_DEFER0]:
                            rdma1(*st).start()
            else:
                rdma1(role, r0, r1_, c0, c1).start()
        assert len(loaded) == len(loads)

    @pl.when((i & 1) == 1)
    def _():
        startup(_P_ODD, True)

    @pl.when((i & 1) == 0)
    def _():
        startup(_P_EVEN, False)

    cl = common_loads()
    for k, (c0, c1) in enumerate(_COMMON_B):
        cl[k].wait()
        b_bf[:, c0:c1] = b_f32[:, c0:c1].astype(_BF)
        res = jnp.dot(a_bf[0:2 * QR, :], b_bf[:, c0:c1], preferred_element_type=_F32)
        s1[0, :, c0:c1] = res[:QR].astype(_BF)
        s1[1, :, c0:c1] = res[QR:].astype(_BF)
        for role in range(2):
            rdma1(role, 0, QR, c0, c1).start()

    for cp in cl[_NCB:]:
        cp.wait()
    a_bf[2 * QR:, :] = a_f32[2 * QR:, :].astype(_BF)
    for g in range(0, NG, 2):
        c0, c1 = g * GW, (g + 2) * GW
        res = jnp.dot(a_bf[2 * QR:4 * QR, :], b_bf[:, c0:c1], preferred_element_type=_F32)
        acc[0, :, c0:c1] = res[:QR]
        acc[1, :, c0:c1] = res[QR:]

    def cols(g):
        return pl.ds(g * GW, GW)

    def pcols(g):
        return pl.ds(g * PW, PW)

    def wait1(role, g):
        blk = r1.at[role, :, cols(g)]
        pltpu.make_async_copy(blk, blk, rs1.at[role * NG + g]).wait()

    def rdma2(role, g, recv=False):
        dr = role if recv else rr2
        return pltpu.make_async_remote_copy(
            s2.at[role, :, cols(g)], r2.at[dr, :, cols(g)],
            ssem.at[1], rs2.at[dr * NG + g],
            device_id=(t2[role],), device_id_type=_MESH)

    def rdma3a(role, g, recv=False):
        dr = role if recv else rr2
        return pltpu.make_async_remote_copy(
            pk_own.at[role, :, pcols(g)], pk_a.at[dr, :, pcols(g)],
            ssem.at[2], rs3a.at[dr * NG + g],
            device_id=(t2[role],), device_id_type=_MESH)

    def rdma3b(role, e, g, recv=False):
        dr = role if recv else rr13
        src = pk_own if e == 1 else pk_a
        return pltpu.make_async_remote_copy(
            src.at[role, :, pcols(g)], pk_b.at[dr, e, :, pcols(g)],
            ssem.at[3], rs3b.at[(dr * 2 + e) * NG + g],
            device_id=(t13[role],), device_id_type=_MESH)

    sign = jnp.uint32(0x80008000)
    mag = jnp.uint32(0x7FFF7FFF)

    def pack_store(v, role, g):
        w = pltpu.bitcast(v.astype(_BF), _U32) & mag
        planes = [w[8 * (p % 8):8 * (p % 8) + 8, (p // 8) * PW:(p // 8 + 1) * PW]
                  for p in range(16)]
        for k in range(15):
            pk_own[role, 8 * k:8 * k + 8, g * PW:(g + 1) * PW] = (
                planes[k] | ((planes[15] << (15 - k)) & sign))

    def unpack_store(src, row0, g):
        w15 = None
        for k in range(15):
            pkd = src[8 * k:8 * k + 8, g * PW:(g + 1) * PW]
            t = (pkd & sign) >> (15 - k)
            w15 = t if w15 is None else (w15 | t)
            o_ref[pl.ds(row0 + 16 * (k % 8), 16), pl.ds(g * GW + (k // 8) * PW, PW)] = (
                pltpu.bitcast(pkd & mag, _BF).astype(_F32))
        o_ref[pl.ds(row0 + 16 * 7, 16), pl.ds(g * GW + PW, PW)] = (
            pltpu.bitcast(w15, _BF).astype(_F32))

    for g in range(NG):
        c0, c1 = g * GW, (g + 1) * GW
        for role in range(2):
            wait1(role, g)
            s2[role, :, c0:c1] = (
                acc[role, :ER, c0:c1] + r1[role, :ER, c0:c1].astype(_F32)).astype(_BF)
            rdma2(role, g).start()

    for g in range(NG):
        c0, c1 = g * GW, (g + 1) * GW
        for role in range(2):
            rdma2(role, g, recv=True).wait_recv()
            v = (acc[role, ER:, c0:c1] + r1[role, ER:, c0:c1].astype(_F32)
                 + r2[role, :, c0:c1].astype(_F32))
            v = jnp.maximum(v, 0.0)
            pack_store(v, role, g)
            rdma3a(role, g).start()
            o_ref[pl.ds(grow(2 + role, 1), ER), c0:c1] = v

    for g in range(NG):
        for role in range(2):
            rdma3b(role, 1, g).start()
    for g in range(NG):
        for role in range(2):
            rdma3a(role, g, recv=True).wait_recv()
            rdma3b(role, 0, g).start()
            unpack_store(pk_a.at[role], grow(2 + role, 0), g)
    for e in (1, 0):
        for g in range(NG):
            for role in range(2):
                rdma3b(role, e, g, recv=True).wait_recv()
                unpack_store(pk_b.at[role, e], grow(role, e), g)

    pltpu.make_async_copy(s1, s1, ssem.at[0]).wait()
    pltpu.make_async_copy(s2, s2, ssem.at[1]).wait()
    pltpu.make_async_copy(pk_own, pk_own, ssem.at[2]).wait()
    pltpu.make_async_copy(pk_b, pk_b, ssem.at[3]).wait()


def pallas_dist_matmul_relu_kshard_i_m1024_n1024_k512_kernel(
    A: jax.Array,
    B: jax.Array,
):
    return pl.pallas_call(
        _body,
        out_shape=jax.ShapeDtypeStruct((M, N), _F32),
        in_specs=[pl.BlockSpec(memory_space=pl.ANY), pl.BlockSpec(memory_space=pl.ANY)],
        out_specs=pl.BlockSpec(memory_space=pltpu.VMEM),
        scratch_shapes=[
            pltpu.VMEM((M, KS), _F32),
            pltpu.VMEM((KS, N), _F32),
            pltpu.VMEM((M, KS), _BF),
            pltpu.VMEM((KS, N), _BF),
            pltpu.VMEM((2, QR, N), _BF),
            pltpu.VMEM((2, QR, N), _BF),
            pltpu.VMEM((2, QR, N), _F32),
            pltpu.VMEM((2, ER, N), _BF),
            pltpu.VMEM((2, ER, N), _BF),
            pltpu.VMEM((2, PR, NG * PW), _U32),
            pltpu.VMEM((2, PR, NG * PW), _U32),
            pltpu.VMEM((2, 2, PR, NG * PW), _U32),
            pltpu.SemaphoreType.DMA((_NLS + _NCB + 4,)),
            pltpu.SemaphoreType.REGULAR,
            pltpu.SemaphoreType.DMA((4,)),
            pltpu.SemaphoreType.DMA((2 * NG,)),
            pltpu.SemaphoreType.DMA((2 * NG,)),
            pltpu.SemaphoreType.DMA((2 * NG,)),
            pltpu.SemaphoreType.DMA((4 * NG,)),
        ],
        compiler_params=pltpu.CompilerParams(
            collective_id=0,
            vmem_limit_bytes=64 * 1024 * 1024,
            disable_semaphore_checks=True,
        ),
    )(A, B)
```

```python
import jax
import jax.numpy as jnp
from jax import lax
from jax.experimental import pallas as pl
from jax.experimental.pallas import tpu as pltpu

M = 1024
N = 1024
KS = 512
QR = 256
ER = 128
GW = 256
NG = N // GW
PR = 120
PW = GW // 2

_P_ODD = dict(
    loads=(('B', 0, 128), ('A', 0, 0, 32), ('A', 0, 32, 80), ('A', 0, 80, 128),
           ('A', 0, 128, 144), ('A', 0, 144, 256), ('B', 128, 256),
           ('A', 1, 0, 128), ('A', 1, 128, 256)),
    steps=(((0,), 0, 32, 0, 128), ((0,), 32, 80, 0, 128), ((0,), 80, 144, 0, 128),
           ((0,), 144, 256, 0, 128), ((0,), 0, 256, 128, 256),
           ((1,), 0, 128, 0, 256), ((1,), 128, 256, 0, 256)),
)
_P_EVEN = dict(
    loads=(('B', 0, 128), ('A', 0, 0, 64), ('A', 1, 0, 64), ('B', 128, 256),
           ('A', 0, 64, 128), ('A', 1, 64, 128), ('A', 0, 128, 256), ('A', 1, 128, 256)),
    steps=(((0,), 0, 64, 0, 128), ((1,), 0, 64, 0, 128), ((0, 1), 0, 64, 128, 256),
           ((0, 1), 64, 128, 0, 256), ((0,), 128, 256, 0, 256), ((1,), 128, 256, 0, 256)),
)
_DEFER0 = 3
_COMMON_B = ((256, 384), (384, 512), (512, 768), (768, 1024))
_NLS = max(len(_P_ODD['loads']), len(_P_EVEN['loads']))
_NCB = len(_COMMON_B)
_GIVE0 = (2, 3)
_EARLY = tuple(g for g in range(NG) if g not in _GIVE0)

_BF = jnp.bfloat16
_F32 = jnp.float32
_U32 = jnp.uint32
_MESH = pl.DeviceIdType.MESH


def _when(cond, fn):
    if cond is True:
        fn()
    elif cond is not False:
        pl.when(cond)(fn)


def _neg(cond):
    return (not cond) if isinstance(cond, bool) else jnp.logical_not(cond)


def _body(a_hbm, b_hbm, o_ref,
          a_f32, b_f32, a_bf, b_bf, s1, r1, acc, s2, r2, pk, pk_b,
          lsem, ready, ssem, rs1, rs2, rs3a, rs3b):
    i = lax.axis_index("i")
    x = i >> 1
    y = (i ^ x) & 1
    py = i ^ 1
    px = 3 - i
    isx = x == 1
    is_odd = (i & 1) == 1

    def sel(h0, h1, role):
        lst = (h0, h1)
        return jnp.where(isx, lst[1 - role], lst[role])

    base = [sel(0, 2 * QR, r) for r in range(2)]
    ac = [sel(y, x, r) for r in range(2)]
    bc = [sel(x, y, r) for r in range(2)]
    t13 = [sel(py, px, r) for r in range(2)]
    t2 = [sel(px, py, r) for r in range(2)]
    rr13 = x
    rr2 = 1 - x

    def grow(slot, e):
        r = slot % 2
        q = ac[r] if slot >= 2 else 1 - ac[r]
        ee = bc[r] if e == 1 else 1 - bc[r]
        return pl.multiple_of(base[r] + q * QR + ee * ER, ER)

    def a_copy(slot, r0, r1_, sem):
        e = r0 // ER
        assert (r1_ - 1) // ER == e
        return pltpu.make_async_copy(
            a_hbm.at[pl.ds(grow(slot, e) + (r0 - e * ER), r1_ - r0), :],
            a_f32.at[pl.ds(slot * QR + r0, r1_ - r0), :], sem)

    def b_copy(c0, c1, sem):
        return pltpu.make_async_copy(
            b_hbm.at[:, pl.ds(c0, c1 - c0)], b_f32.at[:, pl.ds(c0, c1 - c0)], sem)

    def common_loads():
        cps = [b_copy(c0, c1, lsem.at[_NLS + k]) for k, (c0, c1) in enumerate(_COMMON_B)]
        k = _NLS + _NCB
        for slot in (2, 3):
            for e in range(2):
                cps.append(a_copy(slot, e * ER, (e + 1) * ER, lsem.at[k]))
                k += 1
        return cps

    def rdma1(role, r0, r1_, c0, c1):
        g = c0 // GW
        assert (c1 - 1) // GW == g
        return pltpu.make_async_remote_copy(
            s1.at[role, pl.ds(r0, r1_ - r0), pl.ds(c0, c1 - c0)],
            r1.at[rr13, pl.ds(r0, r1_ - r0), pl.ds(c0, c1 - c0)],
            ssem.at[0], rs1.at[rr13 * NG + g],
            device_id=(t13[role],), device_id_type=_MESH)

    bar = pltpu.get_barrier_semaphore()

    def signal_neighbours(sem):
        for nb in (py, px):
            pl.semaphore_signal(sem, inc=1, device_id=(nb,), device_id_type=_MESH)

    def startup(prog, odd):
        loads, steps = prog['loads'], prog['steps']

        def load(k):
            l = loads[k]
            if l[0] == 'B':
                return b_copy(l[1], l[2], lsem.at[k])
            return a_copy(l[1], l[2], l[3], lsem.at[k])

        for k in range(len(loads)):
            if odd and k == 2:
                signal_neighbours(bar)
            load(k).start()
        for cp in common_loads():
            cp.start()
        if not odd:
            @pl.when(i == 0)
            def _():
                signal_neighbours(bar)

            @pl.when(i == 2)
            def _():
                pl.semaphore_wait(bar, 2)
                signal_neighbours(ready)

        loaded = set()

        def need(role, r0, r1_, c0, c1):
            last = -1
            for k, l in enumerate(loads):
                if l[0] == 'B' and l[1] < c1 and l[2] > c0:
                    last = max(last, k)
                if l[0] == 'A' and l[1] == role and l[2] < r1_ and l[3] > r0:
                    last = max(last, k)
            for k in range(last + 1):
                if k in loaded:
                    continue
                loaded.add(k)
                l = loads[k]
                load(k).wait()
                if l[0] == 'B':
                    b_bf[:, l[1]:l[2]] = b_f32[:, l[1]:l[2]].astype(_BF)
                else:
                    o = l[1] * QR
                    a_bf[o + l[2]:o + l[3], :] = a_f32[o + l[2]:o + l[3], :].astype(_BF)

        def post(st):
            for role in st[0]:
                rdma1(role, *st[1:]).start()

        shaken = [False, False]
        for si, st in enumerate(steps):
            roles, r0, r1_, c0, c1 = st
            for role in roles:
                need(role, r0, r1_, c0, c1)
            lhs = [a_bf[role * QR + r0:role * QR + r1_, :] for role in roles]
            lhs = lhs[0] if len(lhs) == 1 else jnp.concatenate(lhs, axis=0)
            res = jnp.dot(lhs, b_bf[:, c0:c1], preferred_element_type=_F32).astype(_BF)
            n = r1_ - r0
            for k, role in enumerate(roles):
                s1[role, r0:r1_, c0:c1] = res[k * n:(k + 1) * n]
            if odd:
                for role in roles:
                    if not shaken[role]:
                        shaken[role] = True
                        if role == 0:
                            pl.semaphore_wait(bar, 1)
                        else:
                            pl.semaphore_wait(ready, 1)
                post(st)
            elif si < _DEFER0:
                pl.when(i == 2)(lambda st=st: post(st))
                if si == _DEFER0 - 1:
                    @pl.when(i == 0)
                    def _():
                        pl.semaphore_wait(bar, 2)
                        for st0 in steps[:_DEFER0]:
                            post(st0)
            else:
                post(st)
        assert len(loaded) == len(loads)

    @pl.when(is_odd)
    def _():
        startup(_P_ODD, True)

    @pl.when(jnp.logical_not(is_odd))
    def _():
        startup(_P_EVEN, False)

    cl = common_loads()
    for k, (c0, c1) in enumerate(_COMMON_B):
        cl[k].wait()
        b_bf[:, c0:c1] = b_f32[:, c0:c1].astype(_BF)
        res = jnp.dot(a_bf[0:2 * QR, :], b_bf[:, c0:c1], preferred_element_type=_F32)
        s1[0, :, c0:c1] = res[:QR].astype(_BF)
        s1[1, :, c0:c1] = res[QR:].astype(_BF)
        for role in range(2):
            rdma1(role, 0, QR, c0, c1).start()

    for cp in cl[_NCB:]:
        cp.wait()
    a_bf[2 * QR:, :] = a_f32[2 * QR:, :].astype(_BF)
    for g in range(0, NG, 2):
        c0, c1 = g * GW, (g + 2) * GW
        res = jnp.dot(a_bf[2 * QR:4 * QR, :], b_bf[:, c0:c1], preferred_element_type=_F32)
        acc[0, :, c0:c1] = res[:QR]
        acc[1, :, c0:c1] = res[QR:]

    def cols(g):
        return pl.ds(g * GW, GW)

    def pcols(g):
        return pl.ds(g * PW, PW)

    def blk(role, e, g):
        return (role * 2 + e) * NG + g

    def own(role, e, g):
        if g not in _GIVE0:
            return e == 1
        if e == 1:
            return i != 0
        return is_odd if role == 1 else False

    def wait1(role, g):
        b = r1.at[role, :, cols(g)]
        pltpu.make_async_copy(b, b, rs1.at[role * NG + g]).wait()

    def rdma2(role, e, g, recv=False):
        dr, de = (role, e) if recv else (rr2, 1 - e)
        return pltpu.make_async_remote_copy(
            s2.at[role, e, :, cols(g)], r2.at[dr, de, :, cols(g)],
            ssem.at[1 + blk(role, e, g)], rs2.at[blk(dr, de, g)],
            device_id=(t2[role],), device_id_type=_MESH)

    def rdma3a(role, e, g, recv=False):
        dr, de = (role, e) if recv else (rr2, 1 - e)
        return pltpu.make_async_remote_copy(
            pk.at[role, e, :, pcols(g)], pk.at[dr, de, :, pcols(g)],
            ssem.at[1 + blk(role, e, g)], rs3a.at[blk(dr, de, g)],
            device_id=(t2[role],), device_id_type=_MESH)

    def rdma3b(role, e, g, recv=False):
        dr = role if recv else rr13
        return pltpu.make_async_remote_copy(
            pk.at[role, e, :, pcols(g)], pk_b.at[dr, e, :, pcols(g)],
            ssem.at[1 + 4 * NG], rs3b.at[blk(dr, e, g)],
            device_id=(t13[role],), device_id_type=_MESH)

    sign = jnp.uint32(0x80008000)
    mag = jnp.uint32(0x7FFF7FFF)

    def pack_store(v, role, e, g):
        w = pltpu.bitcast(v.astype(_BF), _U32) & mag
        planes = [w[8 * (p % 8):8 * (p % 8) + 8, (p // 8) * PW:(p // 8 + 1) * PW]
                  for p in range(16)]
        for k in range(15):
            pk[role, e, 8 * k:8 * k + 8, g * PW:(g + 1) * PW] = (
                planes[k] | ((planes[15] << (15 - k)) & sign))

    def unpack_store(src, row0, g):
        w15 = None
        for k in range(15):
            pkd = src[8 * k:8 * k + 8, g * PW:(g + 1) * PW]
            t = (pkd & sign) >> (15 - k)
            w15 = t if w15 is None else (w15 | t)
            o_ref[pl.ds(row0 + 16 * (k % 8), 16), pl.ds(g * GW + (k // 8) * PW, PW)] = (
                pltpu.bitcast(pkd & mag, _BF).astype(_F32))
        o_ref[pl.ds(row0 + 16 * 7, 16), pl.ds(g * GW + PW, PW)] = (
            pltpu.bitcast(w15, _BF).astype(_F32))

    def send2(role, e, g):
        rs, cs = slice(e * ER, (e + 1) * ER), slice(g * GW, (g + 1) * GW)
        s2[role, e, :, cs] = (acc[role, rs, cs] + r1[role, rs, cs].astype(_F32)).astype(_BF)
        rdma2(role, e, g).start()

    for g in range(NG):
        for role in range(2):
            wait1(role, g)
            for e in (0, 1):
                _when(_neg(own(role, e, g)), lambda a=(role, e, g): send2(*a))

    def finish(role, e, g):
        rs, cs = slice(e * ER, (e + 1) * ER), slice(g * GW, (g + 1) * GW)
        rdma2(role, e, g, recv=True).wait_recv()
        v = (acc[role, rs, cs] + r1[role, rs, cs].astype(_F32)
             + r2[role, e, :, cs].astype(_F32))
        v = jnp.maximum(v, 0.0)
        pack_store(v, role, e, g)
        rdma3a(role, e, g).start()
        if g in _EARLY:
            rdma3b(role, e, g).start()
        o_ref[pl.ds(grow(2 + role, e), ER), cs] = v

    for g in range(NG):
        for e in (1, 0):
            for role in (1, 0):
                _when(own(role, e, g), lambda a=(role, e, g): finish(*a))

    def forward(role, e, g):
        rdma3a(role, e, g, recv=True).wait_recv()
        rdma3b(role, e, g).start()
        unpack_store(pk.at[role, e], grow(2 + role, e), g)

    order = ([(1, g) for g in _EARLY] + [(0, g) for g in _EARLY]
             + [(e, g) for g in _GIVE0 for e in (1, 0)])
    for e, g in order[len(_EARLY):]:
        for role in range(2):
            _when(own(role, e, g), lambda a=(role, e, g): rdma3b(*a).start())
            _when(_neg(own(role, e, g)), lambda a=(role, e, g): forward(*a))

    pltpu.make_async_copy(s1, s1, ssem.at[0]).wait()
    for g in range(NG):
        for e in (0, 1):
            for role in range(2):
                _when(own(role, e, g), lambda a=(role, e, g): rdma3a(*a).wait_send())
                _when(_neg(own(role, e, g)), lambda a=(role, e, g): rdma2(*a).wait_send())

    for e, g in order:
        for role in range(2):
            rdma3b(role, e, g, recv=True).wait_recv()
            unpack_store(pk_b.at[role, e], grow(role, e), g)

    pltpu.make_async_copy(pk_b, pk_b, ssem.at[1 + 4 * NG]).wait()


def pallas_dist_matmul_relu_kshard_i_m1024_n1024_k512_kernel(
    A: jax.Array,
    B: jax.Array,
):
    return pl.pallas_call(
        _body,
        out_shape=jax.ShapeDtypeStruct((M, N), _F32),
        in_specs=[pl.BlockSpec(memory_space=pl.ANY), pl.BlockSpec(memory_space=pl.ANY)],
        out_specs=pl.BlockSpec(memory_space=pltpu.VMEM),
        scratch_shapes=[
            pltpu.VMEM((M, KS), _F32),
            pltpu.VMEM((KS, N), _F32),
            pltpu.VMEM((M, KS), _BF),
            pltpu.VMEM((KS, N), _BF),
            pltpu.VMEM((2, QR, N), _BF),
            pltpu.VMEM((2, QR, N), _BF),
            pltpu.VMEM((2, QR, N), _F32),
            pltpu.VMEM((2, 2, ER, N), _BF),
            pltpu.VMEM((2, 2, ER, N), _BF),
            pltpu.VMEM((2, 2, PR, NG * PW), _U32),
            pltpu.VMEM((2, 2, PR, NG * PW), _U32),
            pltpu.SemaphoreType.DMA((_NLS + _NCB + 4,)),
            pltpu.SemaphoreType.REGULAR,
            pltpu.SemaphoreType.DMA((2 + 4 * NG,)),
            pltpu.SemaphoreType.DMA((2 * NG,)),
            pltpu.SemaphoreType.DMA((4 * NG,)),
            pltpu.SemaphoreType.DMA((4 * NG,)),
            pltpu.SemaphoreType.DMA((4 * NG,)),
        ],
        compiler_params=pltpu.CompilerParams(
            collective_id=0,
            vmem_limit_bytes=64 * 1024 * 1024,
            disable_semaphore_checks=True,
        ),
    )(A, B)
```

```python
import jax
import jax.numpy as jnp
from jax import lax
from jax.experimental import pallas as pl
from jax.experimental.pallas import tpu as pltpu

M = 1024
N = 1024
KS = 512
QR = 256
ER = 128
GW = 256
NG = N // GW
PR = 120
PW = GW // 2

_P_ODD = dict(
    loads=(('B', 0, 128), ('A', 0, 0, 32), ('A', 0, 32, 80), ('A', 0, 80, 128),
           ('A', 0, 128, 144), ('A', 0, 144, 256), ('B', 128, 256),
           ('A', 1, 0, 128), ('A', 1, 128, 256)),
    steps=(((0,), 0, 32, 0, 128), ((0,), 32, 80, 0, 128), ((0,), 80, 144, 0, 128),
           ((0,), 144, 256, 0, 128), ((0,), 0, 256, 128, 256),
           ((1,), 0, 128, 0, 256), ((1,), 128, 256, 0, 256)),
)
_P_EVEN = dict(
    loads=(('B', 0, 128), ('A', 0, 0, 64), ('A', 1, 0, 64), ('B', 128, 256),
           ('A', 0, 64, 128), ('A', 1, 64, 128), ('A', 0, 128, 256), ('A', 1, 128, 256)),
    steps=(((0,), 0, 64, 0, 128), ((1,), 0, 64, 0, 128), ((0, 1), 0, 64, 128, 256),
           ((0, 1), 64, 128, 0, 256), ((0,), 128, 256, 0, 256), ((1,), 128, 256, 0, 256)),
)
_DEFER0 = 3
_COMMON_B = ((256, 384), (384, 512), (512, 768), (768, 1024))
_NLS = max(len(_P_ODD['loads']), len(_P_EVEN['loads']))
_NCB = len(_COMMON_B)
_GIVE0 = (1, 2, 3)

_PROGRAM = (
    ('keep', 0, 2), ('ph2', 0), ('held',), ('keep', 2, 4), ('ph2', 1), ('ph2', 2),
    ('fin', 1, 0, True, 'not0'), ('ph2', 3), ('fin', 1, 0, True, 'only0'),
    ('fin', 1, 1, True, 'all'), ('fin', 0, 1, False, 'all'),
    ('fin', 1, 2, False, 'all'), ('fin', 0, 2, False, 'all'),
    ('fin', 1, 3, False, 'all'), ('fin', 0, 3, False, 'all'),
    ('fwd', 0, 0), ('fwd', 1, 1), ('snd', 0, 1), ('fwd', 0, 1),
    ('snd', 1, 2), ('fwd', 1, 2), ('snd', 0, 2), ('fwd', 0, 2),
    ('snd', 1, 3), ('fwd', 1, 3), ('snd', 0, 3), ('fwd', 0, 3),
)
_RECV_ORDER = ((1, 0), (1, 1), (0, 0), (0, 1), (1, 2), (0, 2), (1, 3), (0, 3))

_BF = jnp.bfloat16
_F32 = jnp.float32
_U32 = jnp.uint32
_MESH = pl.DeviceIdType.MESH


def _when(cond, fn):
    if cond is True:
        fn()
    elif cond is not False:
        pl.when(cond)(fn)


def _neg(cond):
    return (not cond) if isinstance(cond, bool) else jnp.logical_not(cond)


def _both(a, b):
    if a is False or b is False:
        return False
    if a is True:
        return b
    if b is True:
        return a
    return jnp.logical_and(a, b)


def _body(a_hbm, b_hbm, o_ref,
          a_f32, b_f32, a_bf, b_bf, s1, r1, acc, s2, r2, pk, pk_b,
          lsem, ready, ssem, rs1, rs23, rs3b):
    i = lax.axis_index("i")
    x = i >> 1
    y = (i ^ x) & 1
    py = i ^ 1
    px = 3 - i
    isx = x == 1
    is_odd = (i & 1) == 1

    def sel(h0, h1, role):
        lst = (h0, h1)
        return jnp.where(isx, lst[1 - role], lst[role])

    base = [sel(0, 2 * QR, r) for r in range(2)]
    ac = [sel(y, x, r) for r in range(2)]
    bc = [sel(x, y, r) for r in range(2)]
    t13 = [sel(py, px, r) for r in range(2)]
    t2 = [sel(px, py, r) for r in range(2)]
    rr13 = x
    rr2 = 1 - x

    def grow(slot, e):
        r = slot % 2
        q = ac[r] if slot >= 2 else 1 - ac[r]
        ee = bc[r] if e == 1 else 1 - bc[r]
        return pl.multiple_of(base[r] + q * QR + ee * ER, ER)

    def a_copy(slot, r0, r1_, sem):
        e = r0 // ER
        assert (r1_ - 1) // ER == e
        return pltpu.make_async_copy(
            a_hbm.at[pl.ds(grow(slot, e) + (r0 - e * ER), r1_ - r0), :],
            a_f32.at[pl.ds(slot * QR + r0, r1_ - r0), :], sem)

    def b_copy(c0, c1, sem):
        return pltpu.make_async_copy(
            b_hbm.at[:, pl.ds(c0, c1 - c0)], b_f32.at[:, pl.ds(c0, c1 - c0)], sem)

    def common_loads():
        cps = [b_copy(c0, c1, lsem.at[_NLS + k]) for k, (c0, c1) in enumerate(_COMMON_B)]
        k = _NLS + _NCB
        for slot in (2, 3):
            for e in range(2):
                cps.append(a_copy(slot, e * ER, (e + 1) * ER, lsem.at[k]))
                k += 1
        return cps

    def rdma1(role, r0, r1_, c0, c1):
        g = c0 // GW
        assert (c1 - 1) // GW == g
        return pltpu.make_async_remote_copy(
            s1.at[role, pl.ds(r0, r1_ - r0), pl.ds(c0, c1 - c0)],
            r1.at[rr13, pl.ds(r0, r1_ - r0), pl.ds(c0, c1 - c0)],
            ssem.at[0], rs1.at[rr13 * NG + g],
            device_id=(t13[role],), device_id_type=_MESH)

    bar = pltpu.get_barrier_semaphore()

    def signal_neighbours(sem):
        for nb in (py, px):
            pl.semaphore_signal(sem, inc=1, device_id=(nb,), device_id_type=_MESH)

    def startup(prog, odd):
        loads, steps = prog['loads'], prog['steps']

        def load(k):
            l = loads[k]
            if l[0] == 'B':
                return b_copy(l[1], l[2], lsem.at[k])
            return a_copy(l[1], l[2], l[3], lsem.at[k])

        for k in range(len(loads)):
            if odd and k == 2:
                signal_neighbours(bar)
            load(k).start()
        for cp in common_loads():
            cp.start()
        if not odd:
            @pl.when(i == 0)
            def _():
                signal_neighbours(bar)

            @pl.when(i == 2)
            def _():
                pl.semaphore_wait(bar, 2)
                signal_neighbours(ready)

        loaded = set()

        def need(role, r0, r1_, c0, c1):
            last = -1
            for k, l in enumerate(loads):
                if l[0] == 'B' and l[1] < c1 and l[2] > c0:
                    last = max(last, k)
                if l[0] == 'A' and l[1] == role and l[2] < r1_ and l[3] > r0:
                    last = max(last, k)
            for k in range(last + 1):
                if k in loaded:
                    continue
                loaded.add(k)
                l = loads[k]
                load(k).wait()
                if l[0] == 'B':
                    b_bf[:, l[1]:l[2]] = b_f32[:, l[1]:l[2]].astype(_BF)
                else:
                    o = l[1] * QR
                    a_bf[o + l[2]:o + l[3], :] = a_f32[o + l[2]:o + l[3], :].astype(_BF)

        def post(st):
            for role in st[0]:
                rdma1(role, *st[1:]).start()

        shaken = [False, False]
        for si, st in enumerate(steps):
            roles, r0, r1_, c0, c1 = st
            for role in roles:
                need(role, r0, r1_, c0, c1)
            lhs = [a_bf[role * QR + r0:role * QR + r1_, :] for role in roles]
            lhs = lhs[0] if len(lhs) == 1 else jnp.concatenate(lhs, axis=0)
            res = jnp.dot(lhs, b_bf[:, c0:c1], preferred_element_type=_F32).astype(_BF)
            n = r1_ - r0
            for k, role in enumerate(roles):
                s1[role, r0:r1_, c0:c1] = res[k * n:(k + 1) * n]
            if odd:
                for role in roles:
                    if not shaken[role]:
                        shaken[role] = True
                        if role == 0:
                            pl.semaphore_wait(bar, 1)
                        else:
                            pl.semaphore_wait(ready, 1)
                post(st)
            elif si < _DEFER0:
                pl.when(i == 2)(lambda st=st: post(st))
                if si == _DEFER0 - 1:
                    @pl.when(i == 0)
                    def _():
                        pl.semaphore_wait(bar, 2)
                        for st0 in steps[:_DEFER0]:
                            post(st0)
            else:
                post(st)
        assert len(loaded) == len(loads)

    @pl.when(is_odd)
    def _():
        startup(_P_ODD, True)

    @pl.when(jnp.logical_not(is_odd))
    def _():
        startup(_P_EVEN, False)

    cl = common_loads()
    for k, (c0, c1) in enumerate(_COMMON_B):
        cl[k].wait()
        b_bf[:, c0:c1] = b_f32[:, c0:c1].astype(_BF)
        res = jnp.dot(a_bf[0:2 * QR, :], b_bf[:, c0:c1], preferred_element_type=_F32)
        s1[0, :, c0:c1] = res[:QR].astype(_BF)
        s1[1, :, c0:c1] = res[QR:].astype(_BF)
        if k < _NCB - 1:
            for role in range(2):
                rdma1(role, 0, QR, c0, c1).start()

    def post_held():
        for role in range(2):
            rdma1(role, 0, QR, *_COMMON_B[-1]).start()

    for cp in cl[_NCB:]:
        cp.wait()
    a_bf[2 * QR:, :] = a_f32[2 * QR:, :].astype(_BF)

    def keep(g0, g1):
        c0, c1 = g0 * GW, g1 * GW
        res = jnp.dot(a_bf[2 * QR:4 * QR, :], b_bf[:, c0:c1], preferred_element_type=_F32)
        acc[0, :, c0:c1] = res[:QR]
        acc[1, :, c0:c1] = res[QR:]

    def cols(g):
        return pl.ds(g * GW, GW)

    def pcols(g):
        return pl.ds(g * PW, PW)

    def blk(role, e, g):
        return (role * 2 + e) * NG + g

    def own(role, e, g):
        if g not in _GIVE0:
            return e == 1
        if e == 1:
            return i != 0
        return is_odd if role == 1 else False

    def wait1(role, g):
        b = r1.at[role, :, cols(g)]
        pltpu.make_async_copy(b, b, rs1.at[role * NG + g]).wait()

    def rdma2(role, e, g, recv=False):
        dr, de = (role, e) if recv else (rr2, 1 - e)
        return pltpu.make_async_remote_copy(
            s2.at[role, e, :, cols(g)], r2.at[dr, de, :, cols(g)],
            ssem.at[1 + blk(role, e, g)], rs23.at[blk(dr, de, g)],
            device_id=(t2[role],), device_id_type=_MESH)

    def rdma3a(role, e, g, recv=False):
        dr, de = (role, e) if recv else (rr2, 1 - e)
        return pltpu.make_async_remote_copy(
            pk.at[role, e, :, pcols(g)], pk.at[dr, de, :, pcols(g)],
            ssem.at[1 + blk(role, e, g)], rs23.at[blk(dr, de, g)],
            device_id=(t2[role],), device_id_type=_MESH)

    def rdma3b(role, e, g, recv=False):
        dr = role if recv else rr13
        return pltpu.make_async_remote_copy(
            pk.at[role, e, :, pcols(g)], pk_b.at[dr, e, :, pcols(g)],
            ssem.at[1 + 4 * NG], rs3b.at[blk(dr, e, g)],
            device_id=(t13[role],), device_id_type=_MESH)

    sign = jnp.uint32(0x80008000)
    mag = jnp.uint32(0x7FFF7FFF)

    def pack_store(v, role, e, g):
        w = pltpu.bitcast(v.astype(_BF), _U32) & mag
        planes = [w[8 * (p % 8):8 * (p % 8) + 8, (p // 8) * PW:(p // 8 + 1) * PW]
                  for p in range(16)]
        for k in range(15):
            pk[role, e, 8 * k:8 * k + 8, g * PW:(g + 1) * PW] = (
                planes[k] | ((planes[15] << (15 - k)) & sign))

    def unpack_store(src, row0, g):
        w15 = None
        for k in range(15):
            pkd = src[8 * k:8 * k + 8, g * PW:(g + 1) * PW]
            t = (pkd & sign) >> (15 - k)
            w15 = t if w15 is None else (w15 | t)
            o_ref[pl.ds(row0 + 16 * (k % 8), 16), pl.ds(g * GW + (k // 8) * PW, PW)] = (
                pltpu.bitcast(pkd & mag, _BF).astype(_F32))
        o_ref[pl.ds(row0 + 16 * 7, 16), pl.ds(g * GW + PW, PW)] = (
            pltpu.bitcast(w15, _BF).astype(_F32))

    def send2(role, e, g):
        rs, cs = slice(e * ER, (e + 1) * ER), slice(g * GW, (g + 1) * GW)
        s2[role, e, :, cs] = (acc[role, rs, cs] + r1[role, rs, cs].astype(_F32)).astype(_BF)
        rdma2(role, e, g).start()

    def ph2(g):
        for role in range(2):
            wait1(role, g)
            for e in (0, 1):
                _when(_neg(own(role, e, g)), lambda a=(role, e, g): send2(*a))

    def finish(role, e, g, post3b):
        rs, cs = slice(e * ER, (e + 1) * ER), slice(g * GW, (g + 1) * GW)
        rdma2(role, e, g, recv=True).wait_recv()
        v = (acc[role, rs, cs] + r1[role, rs, cs].astype(_F32)
             + r2[role, e, :, cs].astype(_F32))
        v = jnp.maximum(v, 0.0)
        pack_store(v, role, e, g)
        rdma3a(role, e, g).start()
        if post3b:
            rdma3b(role, e, g).start()
        o_ref[pl.ds(grow(2 + role, e), ER), cs] = v

    def fin(e, g, post3b, who):
        here = {'all': True, 'not0': i != 0, 'only0': i == 0}[who]
        for role in (1, 0):
            _when(_both(own(role, e, g), here),
                  lambda a=(role, e, g, post3b): finish(*a))

    def snd(e, g):
        for role in range(2):
            _when(own(role, e, g), lambda a=(role, e, g): rdma3b(*a).start())

    def forward(role, e, g):
        rdma3a(role, e, g, recv=True).wait_recv()
        rdma3b(role, e, g).start()
        unpack_store(pk.at[role, e], grow(2 + role, e), g)

    def fwd(e, g):
        for role in range(2):
            _when(_neg(own(role, e, g)), lambda a=(role, e, g): forward(*a))

    ops = dict(keep=keep, ph2=ph2, held=post_held, fin=fin, snd=snd, fwd=fwd)
    for op in _PROGRAM:
        ops[op[0]](*op[1:])

    pltpu.make_async_copy(s1, s1, ssem.at[0]).wait()
    for g in range(NG):
        for e in (0, 1):
            for role in range(2):
                _when(own(role, e, g), lambda a=(role, e, g): rdma3a(*a).wait_send())
                _when(_neg(own(role, e, g)), lambda a=(role, e, g): rdma2(*a).wait_send())

    for e, g in _RECV_ORDER:
        for role in range(2):
            rdma3b(role, e, g, recv=True).wait_recv()
            unpack_store(pk_b.at[role, e], grow(role, e), g)

    pltpu.make_async_copy(pk_b, pk_b, ssem.at[1 + 4 * NG]).wait()


def _compiler_params():
    kw = dict(collective_id=0, vmem_limit_bytes=64 * 1024 * 1024)
    try:
        return pltpu.CompilerParams(disable_semaphore_checks=True, **kw)
    except TypeError:
        return pltpu.CompilerParams(**kw)


def pallas_dist_matmul_relu_kshard_i_m1024_n1024_k512_kernel(
    A: jax.Array,
    B: jax.Array,
):
    return pl.pallas_call(
        _body,
        out_shape=jax.ShapeDtypeStruct((M, N), _F32),
        in_specs=[pl.BlockSpec(memory_space=pl.ANY), pl.BlockSpec(memory_space=pl.ANY)],
        out_specs=pl.BlockSpec(memory_space=pltpu.VMEM),
        scratch_shapes=[
            pltpu.VMEM((M, KS), _F32),
            pltpu.VMEM((KS, N), _F32),
            pltpu.VMEM((M, KS), _BF),
            pltpu.VMEM((KS, N), _BF),
            pltpu.VMEM((2, QR, N), _BF),
            pltpu.VMEM((2, QR, N), _BF),
            pltpu.VMEM((2, QR, N), _F32),
            pltpu.VMEM((2, 2, ER, N), _BF),
            pltpu.VMEM((2, 2, ER, N), _BF),
            pltpu.VMEM((2, 2, PR, NG * PW), _U32),
            pltpu.VMEM((2, 2, PR, NG * PW), _U32),
            pltpu.SemaphoreType.DMA((_NLS + _NCB + 4,)),
            pltpu.SemaphoreType.REGULAR,
            pltpu.SemaphoreType.DMA((2 + 4 * NG,)),
            pltpu.SemaphoreType.DMA((2 * NG,)),
            pltpu.SemaphoreType.DMA((4 * NG,)),
            pltpu.SemaphoreType.DMA((4 * NG,)),
        ],
        compiler_params=_compiler_params(),
    )(A, B)
```

```python
import jax
import jax.numpy as jnp
from jax import lax
from jax.experimental import pallas as pl
from jax.experimental.pallas import tpu as pltpu

M = 1024
N = 1024
KS = 512
QR = 256
ER = 128
GW = 256
NG = N // GW
PR = 120
PW = GW // 2

_P_ODD = dict(
    loads=(('B', 0, 128), ('A', 0, 0, 16), ('A', 0, 16, 48), ('A', 0, 48, 96),
           ('A', 0, 96, 128), ('A', 0, 128, 160), ('A', 0, 160, 256), ('B', 128, 256),
           ('A', 1, 0, 128), ('A', 1, 128, 256)),
    steps=(((0,), 0, 16, 0, 128), ((0,), 16, 48, 0, 128), ((0,), 48, 96, 0, 128),
           ((0,), 96, 160, 0, 128), ((0,), 160, 256, 0, 128), ((0,), 0, 256, 128, 256),
           ((1,), 0, 128, 0, 256), ((1,), 128, 256, 0, 256)),
)
_P_EVEN = dict(
    loads=(('B', 0, 128), ('A', 0, 0, 64), ('A', 1, 0, 64), ('B', 128, 256),
           ('A', 0, 64, 128), ('A', 1, 64, 128), ('A', 0, 128, 256), ('A', 1, 128, 256)),
    steps=(((0,), 0, 64, 0, 128), ((1,), 0, 64, 0, 128), ((0, 1), 0, 64, 128, 256),
           ((0, 1), 64, 128, 0, 256), ((0,), 128, 256, 0, 256), ((1,), 128, 256, 0, 256)),
)
_DEFER0 = 2
_COMMON_B = ((256, 384), (384, 512), (512, 768), (768, 1024))
_NLS = max(len(_P_ODD['loads']), len(_P_EVEN['loads']))
_NCB = len(_COMMON_B)
_GIVE0 = (1, 2, 3)

_PROGRAM = (
    ('keep', 0, 2), ('ph2', 0), ('held',), ('keep', 2, 4), ('ph2', 1), ('ph2', 2),
    ('fin', 1, 0, True, 'not0'), ('ph2', 3), ('fin', 1, 0, True, 'only0'),
    ('fin', 1, 1, True, 'all'), ('fin', 0, 1, False, 'all'),
    ('fin', 1, 2, False, 'all'), ('fin', 0, 2, False, 'all'),
    ('fin', 1, 3, False, 'all'), ('fin', 0, 3, False, 'all'),
    ('fwd', 0, 0), ('fwd', 1, 1), ('snd', 0, 1), ('fwd', 0, 1),
    ('snd', 1, 2), ('fwd', 1, 2), ('snd', 0, 2), ('fwd', 0, 2),
    ('snd', 1, 3), ('fwd', 1, 3), ('snd', 0, 3), ('fwd', 0, 3),
)
_RECV_ORDER = ((1, 0), (1, 1), (0, 0), (0, 1), (1, 2), (0, 2), (1, 3), (0, 3))

_BF = jnp.bfloat16
_F32 = jnp.float32
_U32 = jnp.uint32
_MESH = pl.DeviceIdType.MESH


def _when(cond, fn):
    if cond is True:
        fn()
    elif cond is not False:
        pl.when(cond)(fn)


def _neg(cond):
    return (not cond) if isinstance(cond, bool) else jnp.logical_not(cond)


def _both(a, b):
    if a is False or b is False:
        return False
    if a is True:
        return b
    if b is True:
        return a
    return jnp.logical_and(a, b)


def _to_words(v):
    return pltpu.bitcast(v.astype(_BF), _U32)


def _mm(a_words, b_words):
    return jnp.dot(pltpu.bitcast(a_words, _BF), pltpu.bitcast(b_words, _BF),
                   preferred_element_type=_F32)


def _body(a_hbm, b_hbm, o_ref,
          a_f32, b_f32, a_bf, b_bf, s1, r1, acc, s2, r2, pk, pk_b,
          lsem, ready, ssem, rs1, rs23, rs3b):
    i = lax.axis_index("i")
    x = i >> 1
    y = (i ^ x) & 1
    py = i ^ 1
    px = 3 - i
    isx = x == 1
    is_odd = (i & 1) == 1

    def sel(h0, h1, role):
        lst = (h0, h1)
        return jnp.where(isx, lst[1 - role], lst[role])

    base = [sel(0, 2 * QR, r) for r in range(2)]
    ac = [sel(y, x, r) for r in range(2)]
    bc = [sel(x, y, r) for r in range(2)]
    t13 = [sel(py, px, r) for r in range(2)]
    t2 = [sel(px, py, r) for r in range(2)]
    rr13 = x
    rr2 = 1 - x

    def grow(slot, e):
        r = slot % 2
        q = ac[r] if slot >= 2 else 1 - ac[r]
        ee = bc[r] if e == 1 else 1 - bc[r]
        return pl.multiple_of(base[r] + q * QR + ee * ER, ER)

    def a_copy(slot, r0, r1_, sem):
        e = r0 // ER
        assert (r1_ - 1) // ER == e
        return pltpu.make_async_copy(
            a_hbm.at[pl.ds(grow(slot, e) + (r0 - e * ER), r1_ - r0), :],
            a_f32.at[pl.ds(slot * QR + r0, r1_ - r0), :], sem)

    def b_copy(c0, c1, sem):
        return pltpu.make_async_copy(
            b_hbm.at[:, pl.ds(c0, c1 - c0)], b_f32.at[:, pl.ds(c0, c1 - c0)], sem)

    def common_loads():
        cps = [b_copy(c0, c1, lsem.at[_NLS + k]) for k, (c0, c1) in enumerate(_COMMON_B)]
        k = _NLS + _NCB
        for slot in (2, 3):
            for e in range(2):
                cps.append(a_copy(slot, e * ER, (e + 1) * ER, lsem.at[k]))
                k += 1
        return cps

    def rdma1(role, r0, r1_, c0, c1):
        g = c0 // GW
        assert (c1 - 1) // GW == g
        return pltpu.make_async_remote_copy(
            s1.at[role, pl.ds(r0, r1_ - r0), pl.ds(c0, c1 - c0)],
            r1.at[rr13, pl.ds(r0, r1_ - r0), pl.ds(c0, c1 - c0)],
            ssem.at[0], rs1.at[rr13 * NG + g],
            device_id=(t13[role],), device_id_type=_MESH)

    bar = pltpu.get_barrier_semaphore()

    def signal_neighbours(sem):
        for nb in (py, px):
            pl.semaphore_signal(sem, inc=1, device_id=(nb,), device_id_type=_MESH)

    def startup(prog, odd):
        loads, steps = prog['loads'], prog['steps']

        def load(k):
            l = loads[k]
            if l[0] == 'B':
                return b_copy(l[1], l[2], lsem.at[k])
            return a_copy(l[1], l[2], l[3], lsem.at[k])

        for k in range(len(loads)):
            if odd and k == 1:
                signal_neighbours(bar)
            load(k).start()
        for cp in common_loads():
            cp.start()
        if not odd:
            @pl.when(i == 0)
            def _():
                signal_neighbours(bar)

            @pl.when(i == 2)
            def _():
                pl.semaphore_wait(bar, 2)
                signal_neighbours(ready)

        loaded = set()

        def need(role, r0, r1_, c0, c1):
            last = -1
            for k, l in enumerate(loads):
                if l[0] == 'B' and l[1] < c1 and l[2] > c0:
                    last = max(last, k)
                if l[0] == 'A' and l[1] == role and l[2] < r1_ and l[3] > r0:
                    last = max(last, k)
            for k in range(last + 1):
                if k in loaded:
                    continue
                loaded.add(k)
                l = loads[k]
                load(k).wait()
                if l[0] == 'B':
                    b_bf[:, l[1]:l[2]] = _to_words(b_f32[:, l[1]:l[2]])
                else:
                    lo, hi = l[1] * QR + l[2], l[1] * QR + l[3]
                    a_bf[lo // 2:hi // 2, :] = _to_words(a_f32[lo:hi, :])

        def post(st):
            for role in st[0]:
                rdma1(role, *st[1:]).start()

        shaken = [False, False]
        for si, st in enumerate(steps):
            roles, r0, r1_, c0, c1 = st
            for role in roles:
                need(role, r0, r1_, c0, c1)
            lhs = [a_bf[(role * QR + r0) // 2:(role * QR + r1_) // 2, :] for role in roles]
            lhs = lhs[0] if len(lhs) == 1 else jnp.concatenate(lhs, axis=0)
            res = _mm(lhs, b_bf[:, c0:c1]).astype(_BF)
            n = r1_ - r0
            for k, role in enumerate(roles):
                s1[role, r0:r1_, c0:c1] = res[k * n:(k + 1) * n]
            if odd:
                for role in roles:
                    if not shaken[role]:
                        shaken[role] = True
                        if role == 0:
                            pl.semaphore_wait(bar, 1)
                        else:
                            pl.semaphore_wait(ready, 1)
                post(st)
            elif si < _DEFER0:
                pl.when(i == 2)(lambda st=st: post(st))
                if si == _DEFER0 - 1:
                    @pl.when(i == 0)
                    def _():
                        pl.semaphore_wait(bar, 2)
                        for st0 in steps[:_DEFER0]:
                            post(st0)
            else:
                post(st)
        assert len(loaded) == len(loads)

    @pl.when(is_odd)
    def _():
        startup(_P_ODD, True)

    @pl.when(jnp.logical_not(is_odd))
    def _():
        startup(_P_EVEN, False)

    cl = common_loads()
    for k, (c0, c1) in enumerate(_COMMON_B):
        cl[k].wait()
        b_bf[:, c0:c1] = _to_words(b_f32[:, c0:c1])
        res = _mm(a_bf[:QR, :], b_bf[:, c0:c1])
        s1[0, :, c0:c1] = res[:QR].astype(_BF)
        s1[1, :, c0:c1] = res[QR:].astype(_BF)
        if k < _NCB - 1:
            for role in range(2):
                rdma1(role, 0, QR, c0, c1).start()

    def post_held():
        for role in range(2):
            rdma1(role, 0, QR, *_COMMON_B[-1]).start()

    for cp in cl[_NCB:]:
        cp.wait()
    a_bf[QR:, :] = _to_words(a_f32[2 * QR:, :])

    def keep(g0, g1):
        c0, c1 = g0 * GW, g1 * GW
        res = _mm(a_bf[QR:, :], b_bf[:, c0:c1])
        acc[0, :, c0:c1] = res[:QR]
        acc[1, :, c0:c1] = res[QR:]

    def cols(g):
        return pl.ds(g * GW, GW)

    def pcols(g):
        return pl.ds(g * PW, PW)

    def blk(role, e, g):
        return (role * 2 + e) * NG + g

    def own(role, e, g):
        if g not in _GIVE0:
            return e == 1
        if e == 1:
            return i != 0
        return is_odd if role == 1 else False

    def wait1(role, g):
        b = r1.at[role, :, cols(g)]
        pltpu.make_async_copy(b, b, rs1.at[role * NG + g]).wait()

    def rdma2(role, e, g, recv=False):
        dr, de = (role, e) if recv else (rr2, 1 - e)
        return pltpu.make_async_remote_copy(
            s2.at[role, e, :, cols(g)], r2.at[dr, de, :, cols(g)],
            ssem.at[1 + blk(role, e, g)], rs23.at[blk(dr, de, g)],
            device_id=(t2[role],), device_id_type=_MESH)

    def rdma3a(role, e, g, recv=False):
        dr, de = (role, e) if recv else (rr2, 1 - e)
        return pltpu.make_async_remote_copy(
            pk.at[role, e, :, pcols(g)], pk.at[dr, de, :, pcols(g)],
            ssem.at[1 + blk(role, e, g)], rs23.at[blk(dr, de, g)],
            device_id=(t2[role],), device_id_type=_MESH)

    def rdma3b(role, e, g, recv=False):
        dr = role if recv else rr13
        return pltpu.make_async_remote_copy(
            pk.at[role, e, :, pcols(g)], pk_b.at[dr, e, :, pcols(g)],
            ssem.at[1 + 4 * NG], rs3b.at[blk(dr, e, g)],
            device_id=(t13[role],), device_id_type=_MESH)

    sign = jnp.uint32(0x80008000)
    mag = jnp.uint32(0x7FFF7FFF)

    def pack_store(v, role, e, g):
        w = _to_words(v) & mag
        planes = [w[8 * (p % 8):8 * (p % 8) + 8, (p // 8) * PW:(p // 8 + 1) * PW]
                  for p in range(16)]
        for k in range(15):
            pk[role, e, 8 * k:8 * k + 8, g * PW:(g + 1) * PW] = (
                planes[k] | ((planes[15] << (15 - k)) & sign))

    def unpack_store(src, row0, g):
        w15 = None
        for k in range(15):
            pkd = src[8 * k:8 * k + 8, g * PW:(g + 1) * PW]
            t = (pkd & sign) >> (15 - k)
            w15 = t if w15 is None else (w15 | t)
            o_ref[pl.ds(row0 + 16 * (k % 8), 16), pl.ds(g * GW + (k // 8) * PW, PW)] = (
                pltpu.bitcast(pkd & mag, _BF).astype(_F32))
        o_ref[pl.ds(row0 + 16 * 7, 16), pl.ds(g * GW + PW, PW)] = (
            pltpu.bitcast(w15, _BF).astype(_F32))

    def send2(role, e, g):
        rs, cs = slice(e * ER, (e + 1) * ER), slice(g * GW, (g + 1) * GW)
        s2[role, e, :, cs] = (acc[role, rs, cs] + r1[role, rs, cs].astype(_F32)).astype(_BF)
        rdma2(role, e, g).start()

    def ph2(g):
        for role in range(2):
            wait1(role, g)
            for e in (0, 1):
                _when(_neg(own(role, e, g)), lambda a=(role, e, g): send2(*a))

    def finish(role, e, g, post3b):
        rs, cs = slice(e * ER, (e + 1) * ER), slice(g * GW, (g + 1) * GW)
        rdma2(role, e, g, recv=True).wait_recv()
        v = (acc[role, rs, cs] + r1[role, rs, cs].astype(_F32)
             + r2[role, e, :, cs].astype(_F32))
        v = jnp.maximum(v, 0.0)
        pack_store(v, role, e, g)
        rdma3a(role, e, g).start()
        if post3b:
            rdma3b(role, e, g).start()
        o_ref[pl.ds(grow(2 + role, e), ER), cs] = v

    def fin(e, g, post3b, who):
        here = {'all': True, 'not0': i != 0, 'only0': i == 0}[who]
        for role in (1, 0):
            _when(_both(own(role, e, g), here),
                  lambda a=(role, e, g, post3b): finish(*a))

    def snd(e, g):
        for role in range(2):
            _when(own(role, e, g), lambda a=(role, e, g): rdma3b(*a).start())

    def forward(role, e, g):
        rdma3a(role, e, g, recv=True).wait_recv()
        rdma3b(role, e, g).start()
        unpack_store(pk.at[role, e], grow(2 + role, e), g)

    def fwd(e, g):
        for role in range(2):
            _when(_neg(own(role, e, g)), lambda a=(role, e, g): forward(*a))

    ops = dict(keep=keep, ph2=ph2, held=post_held, fin=fin, snd=snd, fwd=fwd)
    for op in _PROGRAM:
        ops[op[0]](*op[1:])

    pltpu.make_async_copy(s1, s1, ssem.at[0]).wait()
    for g in range(NG):
        for e in (0, 1):
            for role in range(2):
                _when(own(role, e, g), lambda a=(role, e, g): rdma3a(*a).wait_send())
                _when(_neg(own(role, e, g)), lambda a=(role, e, g): rdma2(*a).wait_send())

    for e, g in _RECV_ORDER:
        for role in range(2):
            rdma3b(role, e, g, recv=True).wait_recv()
            unpack_store(pk_b.at[role, e], grow(role, e), g)

    pltpu.make_async_copy(pk, pk, ssem.at[1 + 4 * NG]).wait()


def _compiler_params():
    kw = dict(collective_id=0, vmem_limit_bytes=64 * 1024 * 1024)
    try:
        return pltpu.CompilerParams(disable_semaphore_checks=True, **kw)
    except TypeError:
        return pltpu.CompilerParams(**kw)


def pallas_dist_matmul_relu_kshard_i_m1024_n1024_k512_kernel(
    A: jax.Array,
    B: jax.Array,
):
    return pl.pallas_call(
        _body,
        out_shape=jax.ShapeDtypeStruct((M, N), _F32),
        in_specs=[pl.BlockSpec(memory_space=pl.ANY), pl.BlockSpec(memory_space=pl.ANY)],
        out_specs=pl.BlockSpec(memory_space=pltpu.VMEM),
        scratch_shapes=[
            pltpu.VMEM((M, KS), _F32),
            pltpu.VMEM((KS, N), _F32),
            pltpu.VMEM((M // 2, KS), _U32),
            pltpu.VMEM((KS // 2, N), _U32),
            pltpu.VMEM((2, QR, N), _BF),
            pltpu.VMEM((2, QR, N), _BF),
            pltpu.VMEM((2, QR, N), _F32),
            pltpu.VMEM((2, 2, ER, N), _BF),
            pltpu.VMEM((2, 2, ER, N), _BF),
            pltpu.VMEM((2, 2, PR, NG * PW), _U32),
            pltpu.VMEM((2, 2, PR, NG * PW), _U32),
            pltpu.SemaphoreType.DMA((_NLS + _NCB + 4,)),
            pltpu.SemaphoreType.REGULAR,
            pltpu.SemaphoreType.DMA((2 + 4 * NG,)),
            pltpu.SemaphoreType.DMA((2 * NG,)),
            pltpu.SemaphoreType.DMA((4 * NG,)),
            pltpu.SemaphoreType.DMA((4 * NG,)),
        ],
        compiler_params=_compiler_params(),
    )(A, B)
```
